```python
import numpy as np
kernel_name = 'dist_attn_cross_mha_kvrep_htp_ss_b1_sq512_skv2048_d1024_hq8_dh128'

def setup_inputs():
    x = np.random.randn(1, 2048, 1024).astype(np.float32)
    Wq = np.random.randn(1024, 4096).astype(np.float32) * 0.02
    K_ext = np.random.randn(1, 2048, 32, 128).astype(np.float32)
    V_ext = np.random.randn(1, 2048, 32, 128).astype(np.float32)
    Wo = np.random.randn(4096, 1024).astype(np.float32) * 0.02
    return {'x': x, 'Wq': Wq, 'K_ext': K_ext, 'V_ext': V_ext, 'Wo': Wo}

def reference(x, Wq, K_ext, V_ext, Wo):
    B, Sq, Hq, Hkv, Dh = (1, 2048, 32, 32, 128)
    Q = (x @ Wq).reshape(B, Sq, Hq, Dh)
    K, V = (K_ext, V_ext)
    Skv = K.shape[1]
    out = np.zeros((B, Sq, Hq, Dh), dtype=np.float32)
    m = np.full((B, Hq, Sq, 1), -np.inf, dtype=np.float32)
    l = np.zeros((B, Hq, Sq, 1), dtype=np.float32)
    for j0 in range(0, Skv, 1024):
        Kj = K[:, j0:j0 + 1024].copy()
        Vj = V[:, j0:j0 + 1024].copy()
        sj = np.einsum('bihd,bjhd->bhij', Q, Kj).astype(np.float32) * 0.08838834764831843
        mj = sj.max(axis=-1, keepdims=True)
        m_new = np.maximum(m, mj)
        alpha = np.exp(m - m_new)
        pj = np.exp(sj - m_new)
        l = l * alpha + pj.sum(axis=-1, keepdims=True)
        out = out * alpha.transpose(0, 2, 1, 3) + np.einsum('bhij,bjhd->bihd', pj, Vj)
        m = m_new
    out = (out / l.transpose(0, 2, 1, 3)).reshape(B, Sq, Hq * Dh)
    return out @ Wo
```

```python
import jax
import jax.numpy as jnp
from jax import lax
from jax.experimental import pallas as pl
from jax.experimental.pallas import tpu as pltpu

N_DEV = 4
SQ = 512
D = 1024
H = 8
HG = 4
DH = 128
SKV = 2048
PIECE = 128
TQ = 256
TQ1 = 272
WQC = 128
KC = 1536

_NT = (((1,), (1,)), ((), ()))
_QSCALE = 0.08838834764831843 * 1.4426950408889634
_MESH = pl.DeviceIdType.MESH

bf16 = jnp.bfloat16
f32 = jnp.float32


def _recip(l):
    r = pl.reciprocal(l, approx=True)
    return r * (2.0 - l * r)


def _lane_tile_sum(p):
    acc = p[:, 0:DH]
    for j in range(1, p.shape[1] // DH):
        acc = acc + p[:, j * DH:(j + 1) * DH]
    return acc


def _loop(lo, hi, fn):
    def step(i, carry):
        fn(i)
        return carry
    lax.fori_loop(lo, hi, step, 0)


def _wait_total(buf, sem):
    pltpu.make_async_copy(buf, buf, sem).wait()


def pallas_dist_attn_cross_mha_kvrep_htp_ss_b1_sq512_skv2048_d1024_hq8_dh128_kernel(
    x: jax.Array,
    Wq: jax.Array,
    K_ext: jax.Array,
    V_ext: jax.Array,
    Wo: jax.Array,
):
    def body(x_hbm, wq_hbm, k_hbm, v_hbm, wo_hbm, out_ref,
             x32, wq32, wo32, k32, v32,
             xb, xr, q_acc, qb, o32, l32, on, ys, yr,
             sem_x, sem_xc, sem_wq, sem_k, sem_v, sem_wo,
             xs_sem, xr_sem, ys_sem, yr_sem, relay_sem):
        me = lax.axis_index("i")
        left = lax.rem(me + 3, N_DEV)
        right = lax.rem(me + 1, N_DEV)
        diag = lax.rem(me + 2, N_DEV)
        h0 = me * H

        x_cp0 = pltpu.make_async_copy(x_hbm.at[0, 0:PIECE], x32.at[0:PIECE], sem_x.at[0])
        x_cp1 = pltpu.make_async_copy(x_hbm.at[0, PIECE:TQ], x32.at[PIECE:TQ], sem_x.at[1])

        def xc_cp(c):
            cols = pl.ds(pl.multiple_of(c * WQC, WQC), WQC)
            return pltpu.make_async_copy(x_hbm.at[0, TQ:SQ, cols], x32.at[TQ:SQ, cols], sem_xc.at[c])

        def wq_cp(c):
            rows = pl.ds(pl.multiple_of(c * WQC, WQC), WQC)
            return pltpu.make_async_copy(wq_hbm.at[rows], wq32.at[rows, 0:D], sem_wq.at[c])

        def k_cp(h):
            return pltpu.make_async_copy(k_hbm.at[0, :, h0 + h, :], k32.at[h], sem_k.at[jnp.minimum(h, HG)])

        def v_cp(h):
            return pltpu.make_async_copy(v_hbm.at[0, :, h0 + h, :], v32.at[h], sem_v.at[jnp.minimum(h, HG)])

        wo_cp = pltpu.make_async_copy(wo_hbm, wo32, sem_wo.at[0])

        def chunk_start(c):
            xc_cp(c).start()
            wq_cp(c).start()

        def kv_start(h):
            k_cp(h).start()
            v_cp(h).start()

        def kv_wait(h):
            k_cp(h).wait()
            v_cp(h).wait()

        bar = pltpu.get_barrier_semaphore()
        x_cp0.start()
        pl.semaphore_signal(bar, inc=1, device_id=(left,), device_id_type=_MESH)
        x_cp1.start()
        pl.semaphore_signal(bar, inc=1, device_id=(right,), device_id_type=_MESH)
        _loop(0, D // WQC, chunk_start)

        def x_send(peer, slot, piece, group, n=1):
            return pltpu.make_async_remote_copy(
                src_ref=xb.at[piece:piece + n], dst_ref=xr.at[slot:slot + n],
                send_sem=xs_sem.at[0], recv_sem=xr_sem.at[group],
                device_id=(peer,), device_id_type=_MESH)

        def y_send(peer, slot, g=0):
            return pltpu.make_async_remote_copy(
                src_ref=ys.at[slot], dst_ref=yr.at[slot],
                send_sem=ys_sem.at[g], recv_sem=yr_sem.at[g],
                device_id=(peer,), device_id_type=_MESH)

        def y_send_pair(blk, j):
            sa = 4 * blk + 2 * j
            y_send(jnp.where(blk == 1, diag, left), sa).start()
            y_send(jnp.where(blk == 1, diag, right), sa + 1).start()

        def store_q(b, r0, q):
            q = (q * _QSCALE).astype(bf16)
            for h in range(H):
                qb[b * H + h, pl.ds(r0, q.shape[0]), :] = q[:, h * DH:(h + 1) * DH]

        def attend(u, h, first):
            split = TQ1 if first else TQ
            for r0, r1 in ((0, split), (split, SQ)):
                q = qb[u, r0:r1]
                if first and r0 == 0:
                    s = lax.dot_general(q, k32[h].astype(bf16), _NT, preferred_element_type=f32)
                    p = jnp.exp2(s - jnp.max(s, axis=-1, keepdims=True))
                    o = jnp.dot(p.astype(bf16), v32[h].astype(bf16), preferred_element_type=f32)
                    l = _lane_tile_sum(p)
                else:
                    s0 = lax.dot_general(q, k32[h, :KC].astype(bf16), _NT, preferred_element_type=f32)
                    s1 = lax.dot_general(q, k32[h, KC:].astype(bf16), _NT, preferred_element_type=f32)
                    m0 = jnp.max(s0, axis=-1, keepdims=True)
                    p0 = jnp.exp2(s0 - m0)
                    o0 = jnp.dot(p0.astype(bf16), v32[h, :KC].astype(bf16), preferred_element_type=f32)
                    m1 = jnp.maximum(m0, jnp.max(s1, axis=-1, keepdims=True))
                    alpha = jnp.exp2(m0 - m1)
                    p1 = jnp.exp2(s1 - m1)
                    o1 = jnp.dot(p1.astype(bf16), v32[h, KC:].astype(bf16), preferred_element_type=f32)
                    o = o0 * alpha + o1
                    l = _lane_tile_sum(p0) * alpha + _lane_tile_sum(p1)
                o32[u, r0:r1] = o
                l32[u, r0:r1] = l

        def normalised(b, lo, hi):
            return jnp.concatenate(
                [(o32[b * H + h] * _recip(jnp.sum(l32[b * H + h], axis=-1, keepdims=True))).astype(bf16)
                 for h in range(lo, hi)], axis=1)

        def project(o, lo, hi):
            return jnp.dot(o, wo32[lo * DH:hi * DH, :].astype(bf16), preferred_element_type=f32)

        def remote_partial():
            return project(normalised(0, 0, H), 0, H).astype(bf16).reshape(4, PIECE, D)

        def own_q_chunk(c):
            kv_start(c)
            xc_cp(c).wait()
            wq_cp(c).wait()
            kk = pl.ds(pl.multiple_of(c * WQC, WQC), WQC)
            xb[2:4, :, kk] = x32[TQ:SQ, kk].astype(bf16).reshape(2, PIECE, WQC)
            part = jnp.dot(x32[:, kk].astype(bf16), wq32[kk, 0:D].astype(bf16), preferred_element_type=f32)
            acc = jnp.where(c > 0, q_acc[...], 0.0) + part
            q_acc[...] = acc
            store_q(1, 0, acc)

        def warm(j):
            _wait_total(xr.at[pl.ds(2 * j, 2)], xr_sem.at[j])

            @pl.when(j == 1)
            def _():
                x_send(diag, 4, 0, 2, n=4).start()
                wo_cp.start()

            q = jnp.dot(xr[pl.ds(2 * j, 2)].reshape(TQ, D), wq32[:, 0:D].astype(bf16), preferred_element_type=f32)
            store_q(0, pl.multiple_of(j * TQ, TQ), q)
            kv_wait(j)
            attend(H + j, j, True)

        def startup():
            x_cp0.wait()
            xb[0] = x32[0:PIECE, :].astype(bf16)
            pl.semaphore_wait(bar, 2)
            x_send(right, 0, 0, 0).start()
            x_send(left, 1, 0, 0).start()
            for peer in (left, right):
                pl.semaphore_signal(relay_sem, inc=1, device_id=(peer,), device_id_type=_MESH)
            x_cp1.wait()
            xb[1] = x32[PIECE:TQ, :].astype(bf16)
            x_send(right, 2, 1, 1).start()
            x_send(left, 3, 1, 1).start()
            _loop(0, D // WQC, own_q_chunk)
            pl.semaphore_wait(relay_sem, 2)
            _loop(0, 2, warm)
            kv_wait(2)
            kv_wait(3)
            attend(H + 2, 2, True)
            attend(H + 3, 3, False)

        def final():
            _wait_total(yr.at[0:10], yr_sem.at[0])
            _wait_total(xr, xs_sem.at[0])
            _wait_total(ys.at[0:10], ys_sem.at[0])
            y = out_ref[0] + project(on[:, 2 * DH:HG * DH], 2, HG)
            y = y + project(normalised(1, HG, H), HG, H) + yr[4:8].reshape(SQ, D).astype(f32)
            for p, s in ((0, 0), (1, 2), (2, 8)):
                rows = slice(p * PIECE, (p + 1) * PIECE)
                out_ref[0, rows, :] = y[rows] + yr[s].astype(f32) + yr[s + 1].astype(f32)
            out_ref[0, 3 * PIECE:SQ, :] = y[3 * PIECE:SQ]
            _wait_total(yr.at[10:12], yr_sem.at[1])
            _wait_total(ys.at[10:12], ys_sem.at[1])
            out_ref[0, 3 * PIECE:SQ, :] = (out_ref[0, 3 * PIECE:SQ, :] + yr[10].astype(f32)
                                           + yr[11].astype(f32))

        def phase(ph):
            pl.when(ph == 0)(startup)

            @pl.when(jnp.logical_or(ph == 1, ph == 2))
            def _():
                _wait_total(xr.at[pl.ds(4 * ph, 4)], xr_sem.at[ph + 1])

                @pl.when(ph == 1)
                def _():
                    wo_cp.wait()
                    for p in (2, 3):
                        x_send(right, 4 + 2 * p, p, 3).start()
                        x_send(left, 5 + 2 * p, p, 3).start()

                q = jnp.dot(xr[pl.ds(4 * ph, 4)].reshape(SQ, D), wq32[:, 0:D].astype(bf16),
                            preferred_element_type=f32)
                store_q(0, 0, q)
                on[...] = normalised(1, 0, HG)
                ys[pl.ds(4 * ph - 4, 4)] = remote_partial()
                y_send_pair(ph - 1, 0)
                y_send_pair(ph - 1, 1)

            @pl.when(ph == 3)
            def _():
                out_ref[0] = project(on[:, 0:2 * DH], 0, 2)
                ys[8:12] = remote_partial()
                y_send(left, 8).start()
                y_send(right, 9).start()
                y_send(left, 10, 1).start()
                y_send(right, 11, 1).start()

            own = (ph == 3).astype(jnp.int32)

            def group(g):
                @pl.when(ph < g)
                def _():
                    _wait_total(k32.at[HG:H], sem_k.at[HG])
                    _wait_total(v32.at[HG:H], sem_v.at[HG])

                for j in range(HG):
                    attend(own * H + g * HG + j, g * HG + j, j == 0)

            _loop(own, 2, group)
            pl.when(ph == 3)(final)

        _loop(0, 4, phase)

    return pl.pallas_call(
        body,
        out_shape=jax.ShapeDtypeStruct((1, SQ, D), f32),
        in_specs=[pl.BlockSpec(memory_space=pl.ANY)] * 5,
        out_specs=pl.BlockSpec(memory_space=pltpu.VMEM),
        scratch_shapes=[
            pltpu.VMEM((SQ, D), f32),
            pltpu.VMEM((D, D + DH), f32),
            pltpu.VMEM((D, D), f32),
            pltpu.VMEM((H, SKV, DH), f32),
            pltpu.VMEM((H, SKV, DH), f32),
            pltpu.VMEM((4, PIECE, D), bf16),
            pltpu.VMEM((12, PIECE, D), bf16),
            pltpu.VMEM((SQ, D), f32),
            pltpu.VMEM((2 * H, SQ, DH), bf16),
            pltpu.VMEM((2 * H, SQ, DH), f32),
            pltpu.VMEM((2 * H, SQ, DH), f32),
            pltpu.VMEM((SQ, HG * DH), bf16),
            pltpu.VMEM((12, PIECE, D), bf16),
            pltpu.VMEM((12, PIECE, D), bf16),
            pltpu.SemaphoreType.DMA((2,)),
            pltpu.SemaphoreType.DMA((D // WQC,)),
            pltpu.SemaphoreType.DMA((D // WQC,)),
            pltpu.SemaphoreType.DMA((HG + 1,)),
            pltpu.SemaphoreType.DMA((HG + 1,)),
            pltpu.SemaphoreType.DMA((1,)),
            pltpu.SemaphoreType.DMA((1,)),
            pltpu.SemaphoreType.DMA((4,)),
            pltpu.SemaphoreType.DMA((2,)),
            pltpu.SemaphoreType.DMA((2,)),
            pltpu.SemaphoreType.REGULAR,
        ],
        compiler_params=pltpu.CompilerParams(
            collective_id=0, vmem_limit_bytes=100 * 1024 * 1024,
            disable_semaphore_checks=True, disable_bounds_checks=True),
    )(x, Wq, K_ext, V_ext, Wo)
```
